```python
import numpy as np

kernel_name = "dist_moe_shared_ep_outshard_n512_d256_e2_h512"

def setup_inputs():
    x = np.random.randn(512, 256).astype(np.float32)
    router_W = np.random.randn(256, 8).astype(np.float32) * 0.1
    scores64 = x.astype(np.float64) @ router_W.astype(np.float64)
    route_idx = np.argsort(-scores64, axis=-1)[:, :1].astype(np.int32)
    expert_W = np.random.randn(8, 256, 512).astype(np.float32) * 0.02
    shared_W = np.random.randn(256, 512).astype(np.float32) * 0.02
    return {"x": x, "router_W": router_W, "route_idx": route_idx, "expert_W": expert_W, "shared_W": shared_W}

def reference(x, router_W, route_idx, expert_W, shared_W):
    scores = x @ router_W
    s_max = scores.max(axis=-1, keepdims=True)
    probs = np.exp(scores - s_max)
    probs = probs / probs.sum(axis=-1, keepdims=True)
    shared = x @ shared_W
    out = np.zeros((512, 512), dtype=np.float32)
    for i in range(512):
        e = int(route_idx[i, 0])
        out[i] = shared[i] + probs[i, e] * (x[i] @ expert_W[e])
    return out
```

```python
import jax
import jax.numpy as jnp
from jax import lax
from jax.experimental import pallas as pl
from jax.experimental.pallas import tpu as pltpu

N_TOK = 512
D = 256
H = 512
N_DEV = 4
TPB = N_TOK // N_DEV
LANES = 128
BF16 = jnp.bfloat16
U32 = jnp.uint32
MESH = pl.DeviceIdType.MESH
CNT0 = 8 * TPB
STAGE_W = CNT0 + LANES
ORDER = (2, 1, 3, 0)
LOG_UNROLL = 2
UNROLL = 1 << LOG_UNROLL
SCOPES = True


def _scope(name):
    return jax.named_scope(name)


def _pack_bf16_pair(lo, hi):
    lo_bits = lax.bitcast_convert_type(lo.astype(BF16).astype(jnp.float32), U32)
    hi_bits = lax.bitcast_convert_type(hi.astype(BF16).astype(jnp.float32), U32)
    return (lo_bits >> 16) | hi_bits


def _unpack_bf16_pair(w):
    lo = lax.bitcast_convert_type(w << 16, jnp.float32)
    hi = lax.bitcast_convert_type(w & jnp.uint32(0xFFFF0000), jnp.float32)
    return lo, hi


def _build_lists(idx4, me):
    a = jnp.concatenate([idx4, idx4], axis=0)
    sub = lax.broadcasted_iota(jnp.int32, (8, TPB), 0)
    lane8 = lax.broadcasted_iota(jnp.int32, (8, TPB), 1)
    mask = a == (2 * me + (sub >= 4).astype(jnp.int32))
    tr = lax.broadcasted_iota(jnp.int32, (TPB, TPB), 0)
    tc = lax.broadcasted_iota(jnp.int32, (TPB, TPB), 1)
    upper = (tr < tc).astype(BF16)
    rank = jnp.dot(mask.astype(jnp.float32).astype(BF16), upper, preferred_element_type=jnp.float32)
    enc_t = jnp.transpose(jnp.where(mask, rank, -1.0))
    lane = tc.astype(jnp.float32)
    ostack = jnp.concatenate([(enc_t[:, q:q + 1] == lane).astype(BF16) for q in range(8)], axis=1)
    tv = lane8.astype(BF16)
    lists = jnp.dot(tv, ostack, preferred_element_type=jnp.float32).astype(jnp.int32)
    valid = jnp.where(tc < 8, jnp.pad(enc_t, ((0, 0), (0, TPB - 8))), -1.0) >= 0.0
    counts = jnp.dot(jnp.ones((8, TPB), BF16), valid.astype(BF16),
                     preferred_element_type=jnp.float32).astype(jnp.int32)
    return lists, counts


def pallas_dist_moe_shared_ep_outshard_n512_d256_e2_h512_kernel(x, router_W, route_idx, expert_W, shared_W):
    rw_t = router_W.T
    idx4 = route_idx.reshape(N_DEV, TPB)
    R3 = 3 * TPB

    def body(idx_hbm, x_hbm, rwt_hbm, ew_hbm, sw_hbm, out_ref,
             idx_v, xv, xb, wv, swv, rwv, send_buf, recv_buf, stage, lsm,
             ld_sems, send_sem, recv_sem, ack_sem):
        me = lax.axis_index("i")
        peers = [(me + d) % N_DEV for d in (1, 2, 3)]
        blk = [(me + d) % N_DEV for d in ORDER]

        bar = pltpu.get_barrier_semaphore()
        for p in peers:
            pl.semaphore_signal(bar, inc=1, device_id=(p,), device_id_type=MESH)

        def load(src, dst, i):
            cp = pltpu.make_async_copy(src, dst, ld_sems.at[i])
            cp.start()
            return cp

        def load_x(j):
            r0 = pl.multiple_of(blk[j] * TPB, TPB)
            return load(x_hbm.at[pl.ds(r0, TPB), :], xv.at[pl.ds(TPB * j, TPB), :], 1 + j)

        with _scope("issue_loads"):
            cp_idx = load(idx_hbm, idx_v, 0)
            cp_x = [load_x(j) for j in range(3)]
            cp_w = [[load(ew_hbm.at[e, :, pl.ds(2 * LANES * c, 2 * LANES)], wv.at[e, :, pl.ds(2 * LANES * c, 2 * LANES)], 5 + 2 * e + c)
                     for c in range(2)] for e in range(2)]
            cp_x.append(load_x(3))
            cp_rw = load(rwt_hbm, rwv, 9)
            cp_sw = load(sw_hbm, swv, 10)

        with _scope("lists"):
            cp_idx.wait()
            lists, counts = _build_lists(idx_v[...], me)
            stage[:, pl.ds(0, CNT0)] = lists
            stage[:, pl.ds(CNT0, LANES)] = counts
            cp_l = pltpu.make_async_copy(stage.at[pl.ds(0, 1), :], lsm, ld_sems.at[11])
            cp_l.start()

        with _scope("x_cast"):
            for j in range(3):
                cp_x[j].wait()
                xb[pl.ds(TPB * j, TPB), :] = xv[pl.ds(TPB * j, TPB), :].astype(BF16)

        def send_group(e, j):
            k = blk[j]
            q = 4 * e + k
            n = lsm[0, CNT0 + q]
            base = TPB * q
            src0 = TPB * j

            def issue(tl2):
                pltpu.make_async_remote_copy(
                    src_ref=send_buf.at[e, :, pl.ds(src0 + tl2, 1), :],
                    dst_ref=recv_buf.at[:, pl.ds(tl2, 1), :],
                    send_sem=send_sem, recv_sem=recv_sem,
                    device_id=(k,), device_id_type=MESH,
                ).start()

            def body_full(it, c):
                i0 = base + UNROLL * it
                tl2 = [lsm[0, i0 + u] for u in range(UNROLL)]
                for u in range(UNROLL):
                    issue(tl2[u])
                return c

            def body_one(i, c):
                issue(lsm[0, base + i])
                return c

            nfull = lax.shift_right_logical(n, LOG_UNROLL)
            lax.fori_loop(0, nfull, body_full, 0)
            lax.fori_loop(lax.shift_left(nfull, LOG_UNROLL), n, body_one, 0)
            return n

        def store_half(e, half, r0, rows, y):
            send_buf[e, half, pl.ds(r0, rows), :] = _pack_bf16_pair(y[:, :LANES], y[:, LANES:])

        def expert_half(e, half, r0, rows):
            w = wv[e, :, pl.ds(2 * LANES * half, 2 * LANES)].astype(BF16)
            store_half(e, half, r0, rows, jnp.dot(xb[pl.ds(r0, rows), :], w, preferred_element_type=jnp.float32))

        def expert_full(e, r0, rows):
            y = jnp.dot(xb[pl.ds(r0, rows), :], wv[e].astype(BF16), preferred_element_type=jnp.float32)
            for half in range(2):
                store_half(e, half, r0, rows, y[:, 2 * LANES * half:2 * LANES * (half + 1)])

        n_sent = jnp.int32(0)
        with _scope("expert0"):
            for half in range(2):
                cp_w[0][half].wait()
                expert_half(0, half, 0, R3)
        with _scope("barrier"):
            cp_l.wait()
            pl.semaphore_wait(bar, N_DEV - 1)
            for p in peers:
                pl.semaphore_signal(ack_sem, inc=1, device_id=(p,), device_id_type=MESH)
        with _scope("send0"):
            for j in range(3):
                n_sent = n_sent + send_group(0, j)
        with _scope("expert1"):
            cp_w[1][0].wait()
            cp_w[1][1].wait()
            expert_full(1, 0, R3)
        with _scope("send1"):
            for j in range(3):
                n_sent = n_sent + send_group(1, j)

        with _scope("own_experts"):
            cp_x[3].wait()
            xb[pl.ds(R3, TPB), :] = xv[pl.ds(R3, TPB), :].astype(BF16)
            for e in range(2):
                expert_full(e, R3, TPB)
            for e in range(2):
                n_sent = n_sent + send_group(e, 3)

        with _scope("shared"):
            cp_rw.wait()
            xl = xv[pl.ds(R3, TPB), :]
            scores_t = lax.dot_general(rwv[...], xl, (((1,), (1,)), ((), ())),
                                       precision=lax.Precision.HIGHEST, preferred_element_type=jnp.float32)
            s_max = jnp.max(scores_t, axis=0, keepdims=True)
            ex = jnp.exp(scores_t - s_max)
            probs_t = ex / jnp.sum(ex, axis=0, keepdims=True)
            idx_l = idx_v[pl.ds(me, 1), :]
            onehot = lax.broadcasted_iota(jnp.int32, (8, TPB), 0) == idx_l
            p_t = jnp.sum(jnp.where(onehot, probs_t, 0.0), axis=0, keepdims=True)
            p_col = jnp.transpose(jnp.broadcast_to(p_t, (8, TPB)))[:, 0:1]
            cp_sw.wait()
            shared = jnp.dot(xb[pl.ds(R3, TPB), :], swv[...].astype(BF16), preferred_element_type=jnp.float32)

        with _scope("wait_recv"):
            pltpu.make_async_copy(recv_buf, recv_buf, recv_sem).wait()
        with _scope("combine"):
            for half in range(2):
                ys = _unpack_bf16_pair(recv_buf[half])
                for j in range(2):
                    c = 2 * half + j
                    out_ref[:, pl.ds(LANES * c, LANES)] = shared[:, LANES * c:LANES * (c + 1)] + p_col * ys[j]

        with _scope("drain"):
            b = N_TOK
            while b >= 1:
                @pl.when((n_sent & b) != 0)
                def _(b=b):
                    ref = send_buf.at[0, :, pl.ds(0, b), :]
                    pltpu.make_async_copy(ref, ref, send_sem).wait()
                b //= 2
            pl.semaphore_wait(ack_sem, N_DEV - 1)

    return pl.pallas_call(
        body,
        out_shape=jax.ShapeDtypeStruct((TPB, H), jnp.float32),
        in_specs=[pl.BlockSpec(memory_space=pl.ANY)] * 5,
        out_specs=pl.BlockSpec(memory_space=pltpu.VMEM),
        scratch_shapes=[
            pltpu.VMEM((N_DEV, TPB), jnp.int32),
            pltpu.VMEM((N_TOK, D), jnp.float32),
            pltpu.VMEM((N_TOK, D), BF16),
            pltpu.VMEM((2, D, H), jnp.float32),
            pltpu.VMEM((D, H), jnp.float32),
            pltpu.VMEM((8, D), jnp.float32),
            pltpu.VMEM((2, 2, N_TOK, LANES), U32),
            pltpu.VMEM((2, TPB, LANES), U32),
            pltpu.VMEM((8, STAGE_W), jnp.int32),
            pltpu.SMEM((1, STAGE_W), jnp.int32),
            pltpu.SemaphoreType.DMA((12,)),
            pltpu.SemaphoreType.DMA,
            pltpu.SemaphoreType.DMA,
            pltpu.SemaphoreType.REGULAR,
        ],
        compiler_params=pltpu.CompilerParams(collective_id=0),
    )(idx4, x, rw_t, expert_W, shared_W)
```

```python
import jax
import jax.numpy as jnp
from jax import lax
from jax.experimental import pallas as pl
from jax.experimental.pallas import tpu as pltpu

N_TOK = 512
D = 256
H = 512
N_DEV = 4
TPB = N_TOK // N_DEV
LANES = 128
BF16 = jnp.bfloat16
F32 = jnp.float32
U32 = jnp.uint32
MESH = pl.DeviceIdType.MESH
CNT0 = 8 * TPB
STAGE_W = CNT0 + LANES
ORDER = (2, 1, 3, 0)
R3 = 3 * TPB
LOG_UNROLL = 2
UNROLL = 1 << LOG_UNROLL


def _pack_bf16_pair(lo, hi):
    lo_bits = lax.bitcast_convert_type(lo.astype(BF16).astype(F32), U32)
    hi_bits = lax.bitcast_convert_type(hi.astype(BF16).astype(F32), U32)
    return (lo_bits >> 16) | hi_bits


def _unpack_bf16_pair(w):
    lo = lax.bitcast_convert_type(w << 16, F32)
    hi = lax.bitcast_convert_type(w & jnp.uint32(0xFFFF0000), F32)
    return lo, hi


def _build_routing(idx_rot, me):
    a = jnp.concatenate([idx_rot, idx_rot], axis=0)
    sub = lax.broadcasted_iota(jnp.int32, (8, TPB), 0)
    lane8 = lax.broadcasted_iota(jnp.int32, (8, TPB), 1)
    mask = a == (2 * me + (sub >= 4).astype(jnp.int32))
    maskb = mask.astype(F32).astype(BF16)
    tr = lax.broadcasted_iota(jnp.int32, (TPB, TPB), 0)
    tc = lax.broadcasted_iota(jnp.int32, (TPB, TPB), 1)
    rank = jnp.dot(maskb, (tr < tc).astype(BF16), preferred_element_type=F32)
    enc_t = jnp.transpose(jnp.where(mask, rank, -1.0))
    lane = tc.astype(F32)
    ostack = jnp.concatenate([(enc_t[:, q:q + 1] == lane).astype(BF16) for q in range(8)], axis=1)
    lists = jnp.dot(lane8.astype(BF16), ostack, preferred_element_type=F32).astype(jnp.int32)
    valid = jnp.where(tc < 8, jnp.pad(enc_t, ((0, 0), (0, TPB - 8))), -1.0) >= 0.0
    counts = jnp.dot(jnp.ones((8, TPB), BF16), valid.astype(BF16), preferred_element_type=F32).astype(jnp.int32)
    cnt_b = jnp.dot(maskb, jnp.ones((TPB, TPB), BF16), preferred_element_type=F32)
    s8 = lax.broadcasted_iota(jnp.int32, (8, 8), 0)
    l8 = lax.broadcasted_iota(jnp.int32, (8, 8), 1)
    tri = (((s8 >> 2) == (l8 >> 2)) & (l8 < s8)).astype(BF16)
    off_b = jnp.dot(tri, cnt_b.astype(BF16), preferred_element_type=F32)
    pos = jnp.where(mask, rank + off_b, -1.0)
    return lists, counts, pos


def pallas_dist_moe_shared_ep_outshard_n512_d256_e2_h512_kernel(x, router_W, route_idx, expert_W, shared_W):
    rw_t = router_W.T
    idx4 = route_idx.reshape(N_DEV, TPB)

    def body(idx_hbm, x_hbm, rwt_hbm, ew_hbm, sw_hbm, out_ref,
             idx_v, xv, xb, xg, wv, swv, rwv, send_buf, recv_buf, stage, lsm,
             ld_sems, send_sem, recv_sem, ack_sem):
        me = lax.axis_index("i")
        peers = [(me + d) % N_DEV for d in (1, 2, 3)]
        blk = [(me + d) % N_DEV for d in ORDER]

        bar = pltpu.get_barrier_semaphore()
        for p in peers:
            pl.semaphore_signal(bar, inc=1, device_id=(p,), device_id_type=MESH)

        def load(src, dst, i):
            cp = pltpu.make_async_copy(src, dst, ld_sems.at[i])
            cp.start()
            return cp

        def load_x(j):
            r0 = pl.multiple_of(blk[j] * TPB, TPB)
            return load(x_hbm.at[pl.ds(r0, TPB), :], xv.at[pl.ds(TPB * j, TPB), :], 1 + j)

        cp_idx = load(idx_hbm, idx_v, 0)
        cp_x = [load_x(j) for j in range(3)]
        cp_w = [[load(ew_hbm.at[e, :, pl.ds(2 * LANES * c, 2 * LANES)],
                      wv.at[e, :, pl.ds(2 * LANES * c, 2 * LANES)], 5 + 2 * e + c)
                 for c in range(2)] for e in range(2)]
        cp_x.append(load_x(3))
        cp_rw = load(rwt_hbm, rwv, 9)
        cp_sw = load(sw_hbm, swv, 10)

        cp_idx.wait()
        idx_rot = jnp.concatenate([idx_v[pl.ds(blk[j], 1), :] for j in range(N_DEV)], axis=0)
        lists, counts, pos = _build_routing(idx_rot, me)
        stage[:, pl.ds(0, CNT0)] = lists
        stage[:, pl.ds(CNT0, LANES)] = counts
        cp_l = pltpu.make_async_copy(stage.at[pl.ds(0, 1), :], lsm, ld_sems.at[11])
        cp_l.start()

        for j in range(3):
            cp_x[j].wait()
            xb[pl.ds(TPB * j, TPB), :] = xv[pl.ds(TPB * j, TPB), :].astype(BF16)

        sub_f = lax.broadcasted_iota(jnp.int32, (TPB, TPB), 0).astype(F32)

        def gather_tile(e, tile):
            p = jnp.concatenate([(sub_f + (TPB * tile) == pos[4 * e + j:4 * e + j + 1, :]).astype(BF16)
                                 for j in range(3)], axis=1)
            return jnp.dot(p, xb[pl.ds(0, R3), :], preferred_element_type=F32).astype(BF16)

        def store_half(e, half, r0, rows, y):
            send_buf[e, half, pl.ds(r0, rows), :] = _pack_bf16_pair(y[:, :LANES], y[:, LANES:])

        def expert_half(e, half, lhs, r0, rows):
            w = wv[e, :, pl.ds(2 * LANES * half, 2 * LANES)].astype(BF16)
            store_half(e, half, r0, rows, jnp.dot(lhs, w, preferred_element_type=F32))

        def expert_full(e, lhs, r0, rows):
            y = jnp.dot(lhs, wv[e].astype(BF16), preferred_element_type=F32)
            for half in range(2):
                store_half(e, half, r0, rows, y[:, 2 * LANES * half:2 * LANES * (half + 1)])

        def send_rows(e, q, n, src_of):
            k = blk[q & 3]
            base = TPB * q

            def issue(i, tl):
                pltpu.make_async_remote_copy(
                    src_ref=send_buf.at[e, :, pl.ds(src_of(i, tl), 1), :],
                    dst_ref=recv_buf.at[:, pl.ds(tl, 1), :],
                    send_sem=send_sem, recv_sem=recv_sem,
                    device_id=(k,), device_id_type=MESH,
                ).start()

            def body_full(it, c):
                i0 = UNROLL * it
                tls = [lsm[0, base + i0 + u] for u in range(UNROLL)]
                for u in range(UNROLL):
                    issue(i0 + u, tls[u])
                return c

            def body_one(i, c):
                issue(i, lsm[0, base + i])
                return c

            nfull = lax.shift_right_logical(n, LOG_UNROLL)
            lax.fori_loop(0, nfull, body_full, 0)
            lax.fori_loop(lax.shift_left(nfull, LOG_UNROLL), n, body_one, 0)

        for e in range(2):
            xg[e] = gather_tile(e, 0)

        n_sent = jnp.int32(0)
        for e in range(2):
            for half in range(2):
                cp_w[e][half].wait()
                expert_half(e, half, xg[e], 0, TPB)
            if e == 0:
                cp_l.wait()
                pl.semaphore_wait(bar, N_DEV - 1)
                for p in peers:
                    pl.semaphore_signal(ack_sem, inc=1, device_id=(p,), device_id_type=MESH)
            cnt = [lsm[0, CNT0 + 4 * e + j] for j in range(3)]
            n_e = cnt[0] + cnt[1] + cnt[2]

            def extra_tile(tile, c, e=e):
                expert_full(e, gather_tile(e, tile), pl.multiple_of(tile * TPB, TPB), TPB)
                return c
            lax.fori_loop(1, lax.shift_right_logical(n_e + (TPB - 1), 7), extra_tile, 0)

            seg = jnp.int32(0)
            for j in range(3):
                send_rows(e, 4 * e + j, cnt[j], lambda i, tl, seg=seg: seg + i)
                seg = seg + cnt[j]
            n_sent = n_sent + n_e

        cp_x[3].wait()
        xb[pl.ds(R3, TPB), :] = xv[pl.ds(R3, TPB), :].astype(BF16)
        for e in range(2):
            expert_full(e, xb[pl.ds(R3, TPB), :], R3, TPB)
        for e in range(2):
            n3 = lsm[0, CNT0 + 4 * e + 3]
            send_rows(e, 4 * e + 3, n3, lambda i, tl: R3 + tl)
            n_sent = n_sent + n3

        cp_rw.wait()
        xl = xv[pl.ds(R3, TPB), :]
        scores_t = lax.dot_general(rwv[...], xl, (((1,), (1,)), ((), ())),
                                   precision=lax.Precision.HIGHEST, preferred_element_type=F32)
        s_max = jnp.max(scores_t, axis=0, keepdims=True)
        ex = jnp.exp(scores_t - s_max)
        probs_t = ex / jnp.sum(ex, axis=0, keepdims=True)
        onehot = lax.broadcasted_iota(jnp.int32, (8, TPB), 0) == idx_rot[3:4, :]
        p_t = jnp.sum(jnp.where(onehot, probs_t, 0.0), axis=0, keepdims=True)
        p_col = jnp.transpose(jnp.broadcast_to(p_t, (8, TPB)))[:, 0:1]
        cp_sw.wait()
        shared = jnp.dot(xb[pl.ds(R3, TPB), :], swv[...].astype(BF16), preferred_element_type=F32)

        pltpu.make_async_copy(recv_buf, recv_buf, recv_sem).wait()
        for half in range(2):
            ys = _unpack_bf16_pair(recv_buf[half])
            for j in range(2):
                c = 2 * half + j
                out_ref[:, pl.ds(LANES * c, LANES)] = shared[:, LANES * c:LANES * (c + 1)] + p_col * ys[j]

        b = N_TOK
        while b >= 1:
            @pl.when((n_sent & b) != 0)
            def _(b=b):
                ref = send_buf.at[0, :, pl.ds(0, b), :]
                pltpu.make_async_copy(ref, ref, send_sem).wait()
            b //= 2
        pl.semaphore_wait(ack_sem, N_DEV - 1)

    return pl.pallas_call(
        body,
        out_shape=jax.ShapeDtypeStruct((TPB, H), F32),
        in_specs=[pl.BlockSpec(memory_space=pl.ANY)] * 5,
        out_specs=pl.BlockSpec(memory_space=pltpu.VMEM),
        scratch_shapes=[
            pltpu.VMEM((N_DEV, TPB), jnp.int32),
            pltpu.VMEM((N_TOK, D), F32),
            pltpu.VMEM((N_TOK, D), BF16),
            pltpu.VMEM((2, TPB, D), BF16),
            pltpu.VMEM((2, D, H), F32),
            pltpu.VMEM((D, H), F32),
            pltpu.VMEM((8, D), F32),
            pltpu.VMEM((2, 2, N_TOK, LANES), U32),
            pltpu.VMEM((2, TPB, LANES), U32),
            pltpu.VMEM((8, STAGE_W), jnp.int32),
            pltpu.SMEM((1, STAGE_W), jnp.int32),
            pltpu.SemaphoreType.DMA((12,)),
            pltpu.SemaphoreType.DMA,
            pltpu.SemaphoreType.DMA,
            pltpu.SemaphoreType.REGULAR,
        ],
        compiler_params=pltpu.CompilerParams(collective_id=0),
    )(idx4, x, rw_t, expert_W, shared_W)
```

```python
import jax
import jax.numpy as jnp
from jax import lax
from jax.experimental import pallas as pl
from jax.experimental.pallas import tpu as pltpu

N_TOK = 512
D = 256
H = 512
N_DEV = 4
TPB = N_TOK // N_DEV
LANES = 128
BF16 = jnp.bfloat16
F32 = jnp.float32
U32 = jnp.uint32
MESH = pl.DeviceIdType.MESH
CNT0 = 8 * TPB
STAGE_W = CNT0 + LANES
ORDER = (2, 1, 3, 0)
R3 = 3 * TPB
LOG_UNROLL = 2
UNROLL = 1 << LOG_UNROLL


def _pack_bf16_pair(lo, hi):
    lo_bits = lax.bitcast_convert_type(lo.astype(BF16).astype(F32), U32)
    hi_bits = lax.bitcast_convert_type(hi.astype(BF16).astype(F32), U32)
    return (lo_bits >> 16) | hi_bits


def _unpack_bf16_pair(w):
    lo = lax.bitcast_convert_type(w << 16, F32)
    hi = lax.bitcast_convert_type(w & jnp.uint32(0xFFFF0000), F32)
    return lo, hi


def _build_routing(idx_rot, me):
    a = jnp.concatenate([idx_rot, idx_rot], axis=0)
    sub = lax.broadcasted_iota(jnp.int32, (8, TPB), 0)
    lane8 = lax.broadcasted_iota(jnp.int32, (8, TPB), 1)
    mask = a == (2 * me + (sub >= 4).astype(jnp.int32))
    maskb = mask.astype(F32).astype(BF16)
    tr = lax.broadcasted_iota(jnp.int32, (TPB, TPB), 0)
    tc = lax.broadcasted_iota(jnp.int32, (TPB, TPB), 1)
    rank = jnp.dot(maskb, (tr < tc).astype(BF16), preferred_element_type=F32)
    enc_t = jnp.transpose(jnp.where(mask, rank, -1.0))
    lane = tc.astype(F32)
    ostack = jnp.concatenate([(enc_t[:, q:q + 1] == lane).astype(BF16) for q in range(8)], axis=1)
    lists = jnp.dot(lane8.astype(BF16), ostack, preferred_element_type=F32).astype(jnp.int32)
    valid = jnp.where(tc < 8, jnp.pad(enc_t, ((0, 0), (0, TPB - 8))), -1.0) >= 0.0
    counts = jnp.dot(jnp.ones((8, TPB), BF16), valid.astype(BF16), preferred_element_type=F32).astype(jnp.int32)
    cnt_b = jnp.dot(maskb, jnp.ones((TPB, TPB), BF16), preferred_element_type=F32)
    s8 = lax.broadcasted_iota(jnp.int32, (8, 8), 0)
    l8 = lax.broadcasted_iota(jnp.int32, (8, 8), 1)
    tri = (((s8 >> 2) == (l8 >> 2)) & (l8 < s8)).astype(BF16)
    off_b = jnp.dot(tri, cnt_b.astype(BF16), preferred_element_type=F32)
    pos = jnp.where(mask, rank + off_b, -1.0)
    return lists, counts, pos


def pallas_dist_moe_shared_ep_outshard_n512_d256_e2_h512_kernel(x, router_W, route_idx, expert_W, shared_W):
    rw_t = router_W.T
    idx4 = route_idx.reshape(N_DEV, TPB)

    def body(idx_hbm, x_hbm, rwt_hbm, ew_hbm, sw_hbm, out_ref,
             idx_v, xv, xb, xg, wv, swv, rwv, send_buf, recv_buf, stage, lsm,
             ld_sems, send_sem, recv_sem, ack_sem):
        me = lax.axis_index("i")
        peers = [(me + d) % N_DEV for d in (1, 2, 3)]
        blk = [(me + d) % N_DEV for d in ORDER]

        bar = pltpu.get_barrier_semaphore()
        for p in peers:
            pl.semaphore_signal(bar, inc=1, device_id=(p,), device_id_type=MESH)

        def load(src, dst, i):
            cp = pltpu.make_async_copy(src, dst, ld_sems.at[i])
            cp.start()
            return cp

        def load_x(j):
            r0 = pl.multiple_of(blk[j] * TPB, TPB)
            return load(x_hbm.at[pl.ds(r0, TPB), :], xv.at[pl.ds(TPB * j, TPB), :], 1 + j)

        cp_idx = load(idx_hbm, idx_v, 0)
        cp_x = [load_x(j) for j in range(3)]
        cp_w = [[load(ew_hbm.at[e, :, pl.ds(2 * LANES * c, 2 * LANES)],
                      wv.at[e, :, pl.ds(2 * LANES * c, 2 * LANES)], 5 + 2 * e + c)
                 for c in range(2)] for e in range(2)]
        cp_x.append(load_x(3))
        cp_rw = load(rwt_hbm, rwv, 9)
        cp_sw = load(sw_hbm, swv, 10)

        cp_idx.wait()
        idx_rot = jnp.concatenate([idx_v[pl.ds(blk[j], 1), :] for j in range(N_DEV)], axis=0)
        lists, counts, pos = _build_routing(idx_rot, me)
        stage[:, pl.ds(0, CNT0)] = lists
        stage[:, pl.ds(CNT0, LANES)] = counts
        cp_l = pltpu.make_async_copy(stage.at[pl.ds(0, 1), :], lsm, ld_sems.at[11])
        cp_l.start()

        for j in range(3):
            cp_x[j].wait()
            xb[pl.ds(TPB * j, TPB), :] = xv[pl.ds(TPB * j, TPB), :].astype(BF16)

        sub_f = lax.broadcasted_iota(jnp.int32, (TPB, TPB), 0).astype(F32)

        def gather_tile(e, tile):
            p = jnp.concatenate([(sub_f + (TPB * tile) == pos[4 * e + j:4 * e + j + 1, :]).astype(BF16)
                                 for j in range(3)], axis=1)
            return jnp.dot(p, xb[pl.ds(0, R3), :], preferred_element_type=F32).astype(BF16)

        def store_half(e, half, r0, rows, y):
            send_buf[e, half, pl.ds(r0, rows), :] = _pack_bf16_pair(y[:, :LANES], y[:, LANES:])

        def expert_half(e, half, lhs, r0, rows):
            w = wv[e, :, pl.ds(2 * LANES * half, 2 * LANES)].astype(BF16)
            store_half(e, half, r0, rows, jnp.dot(lhs, w, preferred_element_type=F32))

        def expert_full(e, lhs, r0, rows):
            y = jnp.dot(lhs, wv[e].astype(BF16), preferred_element_type=F32)
            for half in range(2):
                store_half(e, half, r0, rows, y[:, 2 * LANES * half:2 * LANES * (half + 1)])

        def send_rows(e, q, n, src_of):
            k = blk[q & 3]
            base = TPB * q

            def issue(i, tl):
                pltpu.make_async_remote_copy(
                    src_ref=send_buf.at[e, :, pl.ds(src_of(i, tl), 1), :],
                    dst_ref=recv_buf.at[:, pl.ds(tl, 1), :],
                    send_sem=send_sem, recv_sem=recv_sem,
                    device_id=(k,), device_id_type=MESH,
                ).start()

            def body_full(it, c):
                i0 = UNROLL * it
                tls = [lsm[0, base + i0 + u] for u in range(UNROLL)]
                for u in range(UNROLL):
                    issue(i0 + u, tls[u])
                return c

            def body_one(i, c):
                issue(i, lsm[0, base + i])
                return c

            nfull = lax.shift_right_logical(n, LOG_UNROLL)
            lax.fori_loop(0, nfull, body_full, 0)
            lax.fori_loop(lax.shift_left(nfull, LOG_UNROLL), n, body_one, 0)

        for e in range(2):
            xg[e] = gather_tile(e, 0)

        n_sent = jnp.int32(0)
        for e in range(2):
            if e == 0:
                for half in range(2):
                    cp_w[e][half].wait()
                    expert_half(e, half, xg[e], 0, TPB)
            else:
                cp_w[e][0].wait()
                cp_w[e][1].wait()
                expert_full(e, xg[e], 0, TPB)
            if e == 0:
                cp_l.wait()
                pl.semaphore_wait(bar, N_DEV - 1)
                for p in peers:
                    pl.semaphore_signal(ack_sem, inc=1, device_id=(p,), device_id_type=MESH)
            cnt = [lsm[0, CNT0 + 4 * e + j] for j in range(3)]
            n_e = cnt[0] + cnt[1] + cnt[2]

            def extra_tile(tile, c, e=e):
                expert_full(e, gather_tile(e, tile), pl.multiple_of(tile * TPB, TPB), TPB)
                return c
            lax.fori_loop(1, lax.shift_right_logical(n_e + (TPB - 1), 7), extra_tile, 0)

            seg = jnp.int32(0)
            for j in range(3):
                send_rows(e, 4 * e + j, cnt[j], lambda i, tl, seg=seg: seg + i)
                seg = seg + cnt[j]
            n_sent = n_sent + n_e

        cp_x[3].wait()
        xb[pl.ds(R3, TPB), :] = xv[pl.ds(R3, TPB), :].astype(BF16)
        for e in range(2):
            expert_full(e, xb[pl.ds(R3, TPB), :], R3, TPB)
        for e in range(2):
            n3 = lsm[0, CNT0 + 4 * e + 3]
            send_rows(e, 4 * e + 3, n3, lambda i, tl: R3 + tl)
            n_sent = n_sent + n3

        cp_rw.wait()
        xl = xv[pl.ds(R3, TPB), :]
        scores_t = lax.dot_general(rwv[...], xl, (((1,), (1,)), ((), ())),
                                   precision=lax.Precision.HIGHEST, preferred_element_type=F32)
        s_max = jnp.max(scores_t, axis=0, keepdims=True)
        ex = jnp.exp(scores_t - s_max)
        probs_t = ex / jnp.sum(ex, axis=0, keepdims=True)
        onehot = lax.broadcasted_iota(jnp.int32, (8, TPB), 0) == idx_rot[3:4, :]
        p_t = jnp.sum(jnp.where(onehot, probs_t, 0.0), axis=0, keepdims=True)
        p_col = jnp.transpose(jnp.broadcast_to(p_t, (8, TPB)))[:, 0:1]
        cp_sw.wait()
        shared = jnp.dot(xb[pl.ds(R3, TPB), :], swv[...].astype(BF16), preferred_element_type=F32)

        pltpu.make_async_copy(recv_buf, recv_buf, recv_sem).wait()
        for half in range(2):
            ys = _unpack_bf16_pair(recv_buf[half])
            for j in range(2):
                c = 2 * half + j
                out_ref[:, pl.ds(LANES * c, LANES)] = shared[:, LANES * c:LANES * (c + 1)] + p_col * ys[j]

        b = N_TOK
        while b >= 1:
            @pl.when((n_sent & b) != 0)
            def _(b=b):
                ref = send_buf.at[0, :, pl.ds(0, b), :]
                pltpu.make_async_copy(ref, ref, send_sem).wait()
            b //= 2
        pl.semaphore_wait(ack_sem, N_DEV - 1)

    return pl.pallas_call(
        body,
        out_shape=jax.ShapeDtypeStruct((TPB, H), F32),
        in_specs=[pl.BlockSpec(memory_space=pl.ANY)] * 5,
        out_specs=pl.BlockSpec(memory_space=pltpu.VMEM),
        scratch_shapes=[
            pltpu.VMEM((N_DEV, TPB), jnp.int32),
            pltpu.VMEM((N_TOK, D), F32),
            pltpu.VMEM((N_TOK, D), BF16),
            pltpu.VMEM((2, TPB, D), BF16),
            pltpu.VMEM((2, D, H), F32),
            pltpu.VMEM((D, H), F32),
            pltpu.VMEM((8, D), F32),
            pltpu.VMEM((2, 2, N_TOK, LANES), U32),
            pltpu.VMEM((2, TPB, LANES), U32),
            pltpu.VMEM((8, STAGE_W), jnp.int32),
            pltpu.SMEM((1, STAGE_W), jnp.int32),
            pltpu.SemaphoreType.DMA((12,)),
            pltpu.SemaphoreType.DMA,
            pltpu.SemaphoreType.DMA,
            pltpu.SemaphoreType.REGULAR,
        ],
        compiler_params=pltpu.CompilerParams(collective_id=0),
    )(idx4, x, rw_t, expert_W, shared_W)
```
